```python
import numpy as np

kernel_name = "dist_halo_stencil_i_m8192_n1024"

def setup_inputs():
    return {"x": np.random.randn(32768, 1024).astype(np.float32)}

def reference(x: np.ndarray) -> np.ndarray:
    out = np.empty_like(x)
    out[0] = x[0]
    out[-1] = x[-1]
    out[1:-1] = 0.25 * x[:-2] + 0.5 * x[1:-1] + 0.25 * x[2:]
    return out
```

```python
import jax
import jax.numpy as jnp
from jax import lax
from jax.experimental import pallas as pl
from jax.experimental.pallas import tpu as pltpu

N_DEV = 4
SUB, LANES = 8, 128
SEGS = LANES // SUB
PARTS = 4
PAIR = 2

READS = (16, 9, 7, 7, 5, 4, 4, 2, 2)
COLUMN_READS = (5, 2, 1)
EDGE_READ = 5
STAGED_READ = 6
STAGED_SLABS, STAGED_SEGS = 2, 4
UNSTAGE_STEPS = (14, 30)


def pallas_dist_halo_stencil_i_m8192_n1024_kernel(
    x: jax.Array,
):
    m, n = x.shape
    n_col = n // LANES
    n_seg = PARTS * SEGS
    seg_len = m // (SUB * n_seg)
    last = seg_len - 1
    n_step = sum(READS) + STAGED_SLABS
    last_part, tail = divmod(n_step, seg_len)
    tail_seg = last_part * SEGS
    n_staged = len(UNSTAGE_STEPS) + 1
    assert last_part == PARTS - 1 and tail + 1 < last and sum(COLUMN_READS) == n_col

    def needed_at(slab):
        return slab - 1 if slab > last_part * seg_len else max(slab - 2, 0)

    def body(x_hbm, y_ref, buf, stage, read_sems, in_sems, out_sems, send_sems, recv_sems):
        def read(sem, seg, u, count, cols=slice(None), rows=slice(None), segs=SEGS):
            return pltpu.make_async_copy(
                x_hbm.at[pl.ds(seg, segs), pl.ds(u, count), cols, rows],
                buf.at[pl.ds(seg + 1, segs), pl.ds(u, count), cols, rows],
                read_sems.at[sem],
            )

        reads, to_stage, from_stage = [], [], []
        slab = 0
        for i, count in enumerate(READS):
            step, copies = needed_at(slab), []
            if i == EDGE_READ:
                assert step <= last_part * seg_len
                copies.append(read(i, tail_seg, tail, 1, rows=pl.ds(0, 1)))
                copies.append(read(i, tail_seg, last, 1, rows=pl.ds(SUB - 1, 1)))
            if i == STAGED_READ:
                seg, u = slab // seg_len * SEGS, slab % seg_len
                for j in range(n_staged):
                    src = x_hbm.at[pl.ds(seg, STAGED_SEGS), pl.ds(u, STAGED_SLABS)]
                    dst = buf.at[pl.ds(seg + 1, STAGED_SEGS), pl.ds(u, STAGED_SLABS)]
                    to_stage.append(
                        pltpu.make_async_copy(src, stage.at[j], in_sems.at[j])
                    )
                    from_stage.append(
                        pltpu.make_async_copy(stage.at[j], dst, out_sems.at[j])
                    )
                    seg += STAGED_SEGS
                rest = SEGS - n_staged * STAGED_SEGS
                copies.append(read(i, seg, u, STAGED_SLABS, segs=rest))
                staged_step = step
                slab += STAGED_SLABS
            copies.append(read(i, slab // seg_len * SEGS, slab % seg_len, count))
            reads.append((step, copies))
            slab += count

        column_reads = []
        c = 0
        for i, width in enumerate(COLUMN_READS, len(READS)):
            cols = pl.ds(c, width)
            copies = [
                read(i, tail_seg, tail, 1, cols, pl.ds(1, SUB - 1)),
                read(i, tail_seg, tail + 1, last - tail - 1, cols),
                read(i, tail_seg, last, 1, cols, pl.ds(0, SUB - 1)),
            ]
            column_reads.append((range(c, c + width), copies))
            c += width

        for i, (_, copies) in enumerate(reads + column_reads):
            for copy in copies + (to_stage if i == 0 else []):
                copy.start()

        me = lax.axis_index("i")
        left, right = (me + N_DEV - 1) % N_DEV, (me + 1) % N_DEV
        barrier = pltpu.get_barrier_semaphore()
        for peer in (left, right):
            pl.semaphore_signal(
                barrier, inc=1, device_id=(peer,), device_id_type=pl.DeviceIdType.MESH
            )
        first_row = (0, slice(None), pl.ds(0, 1))
        last_row = (last, slice(None), pl.ds(SUB - 1, 1))
        halos = [
            pltpu.make_async_remote_copy(
                x_hbm.at[(src, *row)],
                buf.at[(dst, *row)],
                send_sems.at[i],
                recv_sems.at[i],
                device_id=(peer,),
                device_id_type=pl.DeviceIdType.MESH,
            )
            for i, (src, dst, row, peer) in enumerate(
                [(n_seg - 1, 0, last_row, right), (0, n_seg + 1, first_row, left)]
            )
        ]

        to_stage[0].wait()
        from_stage[0].start()
        pl.semaphore_wait(barrier, 2)
        for copy in halos:
            copy.start()

        sublane = lax.broadcasted_iota(jnp.int32, (1, SUB, LANES), 1)

        def stencil(part, u, c, keep_first=None, keep_last=None, whole=False):
            seg = part * SEGS + 1
            at_top, at_bottom = u == 0, u == last
            above = (
                pl.ds(seg - jnp.where(at_top, 1, 0), SEGS),
                jnp.where(at_top, last, u - 1),
                c,
            )
            below = (
                pl.ds(seg + jnp.where(at_bottom, 1, 0), SEGS),
                jnp.where(at_bottom, 0, u + 1),
                c,
            )
            cur = buf[pl.ds(seg, SEGS), u, c]
            top, bottom = sublane == 0, sublane == SUB - 1
            if whole:
                prev = pltpu.roll(jnp.where(bottom, buf[above], cur), 1, 1)
                nxt = pltpu.roll(jnp.where(top, buf[below], cur), SUB - 1, 1)
            else:
                prev = jnp.where(
                    top, buf[(*above, pl.ds(SUB - 1, 1))], pltpu.roll(cur, 1, 1)
                )
                nxt = jnp.where(
                    bottom, buf[(*below, pl.ds(0, 1))], pltpu.roll(cur, SUB - 1, 1)
                )
            out = 0.25 * prev + 0.5 * cur + 0.25 * nxt
            if keep_first is not None:
                edge = jnp.where(sublane == keep_first, cur[:1], out[:1])
                out = jnp.concatenate([edge, out[1:]])
            if keep_last is not None:
                edge = jnp.where(sublane == keep_last, cur[-1:], out[-1:])
                out = jnp.concatenate([out[:-1], edge])
            row = ((part // PAIR * seg_len + u) * n + c * LANES) * PAIR + part % PAIR
            y_ref[pl.ds(row, LANES, stride=PAIR), :] = out.reshape(LANES, LANES).T

        @pl.loop(0, n_step)
        def sweep(k):
            for step, landing, leaving in zip(UNSTAGE_STEPS, to_stage[1:], from_stage[1:]):

                @pl.when(k == step)
                def _():
                    landing.wait()
                    leaving.start()

            for step, copies in reads + [(last, halos), (staged_step, from_stage)]:

                @pl.when(k == step)
                def _():
                    for copy in copies:
                        copy.wait()

            part = k // seg_len
            u = jnp.where(part == last_part, k, k + 1) % seg_len
            keep = jnp.where(jnp.logical_and(k == last, me == 0), 0, -1)
            for c in range(n_col):
                stencil(part, u, c, keep_first=keep)

        keep = jnp.where(me == N_DEV - 1, SUB - 1, -1)
        for columns, copies in column_reads:
            for copy in copies:
                copy.wait()
            for c in columns:
                for u in range(tail, last):
                    stencil(last_part, u, c, whole=True)
                stencil(last_part, last, c, keep_last=keep)

    tiles = x.reshape(m // SUB, SUB, n_col, LANES).transpose(0, 2, 1, 3)
    y = pl.pallas_call(
        body,
        out_shape=pltpu.VMEM((m * n // LANES, LANES), x.dtype),
        in_specs=[pl.BlockSpec(memory_space=pltpu.HBM)],
        out_specs=pl.BlockSpec(memory_space=pltpu.VMEM),
        scratch_shapes=[
            pltpu.VMEM((n_seg + 2, seg_len, n_col, SUB, LANES), x.dtype),
            pltpu.SMEM((n_staged, STAGED_SEGS, STAGED_SLABS, n_col, SUB, LANES), x.dtype),
            pltpu.SemaphoreType.DMA((len(READS) + len(COLUMN_READS),)),
            pltpu.SemaphoreType.DMA((n_staged,)),
            pltpu.SemaphoreType.DMA((n_staged,)),
            pltpu.SemaphoreType.DMA((2,)),
            pltpu.SemaphoreType.DMA((2,)),
        ],
        compiler_params=pltpu.CompilerParams(
            collective_id=0,
            vmem_limit_bytes=40 * 2**20,
            disable_semaphore_checks=True,
        ),
    )(tiles.reshape(n_seg, seg_len, n_col, SUB, LANES))
    y = y.reshape(PARTS // PAIR, -1, PAIR, LANES).transpose(0, 2, 3, 1)
    y = y.reshape(PARTS, SEGS, SUB, -1).transpose(1, 0, 2, 3)
    y = y.reshape(SEGS, PARTS, SUB, seg_len, n).transpose(1, 0, 3, 2, 4)
    return y.reshape(m, n)
```
